```python
import numpy as np

kernel_name = "dist_mlpseq_tp1d_bs_rep_b64_d1024_h2048"

def setup_inputs():
    x = np.random.randn(256, 1024).astype(np.float32)
    Win0 = np.random.randn(1024, 8192).astype(np.float32)
    Wout0 = np.random.randn(8192, 1024).astype(np.float32)
    Win1 = np.random.randn(1024, 8192).astype(np.float32)
    Wout1 = np.random.randn(8192, 1024).astype(np.float32)
    Win2 = np.random.randn(1024, 8192).astype(np.float32)
    Wout2 = np.random.randn(8192, 1024).astype(np.float32)
    return {"x": x, "Win0": Win0, "Wout0": Wout0, "Win1": Win1, "Wout1": Wout1, "Win2": Win2, "Wout2": Wout2}

def reference(x, Win0, Win1, Win2, Wout0, Wout1, Wout2):
    h = x @ Win0
    h = np.maximum(h, 0.0)
    x = h @ Wout0
    h = x @ Win1
    h = np.maximum(h, 0.0)
    x = h @ Wout1
    h = x @ Win2
    h = np.maximum(h, 0.0)
    x = h @ Wout2
    return x
```

```python
import contextlib
import jax
import jax.numpy as jnp
from jax import lax
from jax.experimental import pallas as pl
from jax.experimental.pallas import tpu as pltpu

MESH = pl.DeviceIdType.MESH
BF = jnp.bfloat16
F32 = jnp.float32
B, D, H, L = 256, 1024, 2048, 3
CW = 128
NC = D // CW

DEF = dict(
    NU=512,
    win=([2048], [1024, 512, 512], [1024, 512, 512]),
    w0=[512, 512], w1=[384, 384, 128, 128], w2=None,
    kp=(1024, 1024), lpar=(2, 2, 2), na=5, lag3=3, tail='a5 t2 b5 s4 a6 t3 b6 s5 a7 t4 b7 s6 t5 s7 g0 t6 t7',
    n3=6, sub6=2, sub=2, odt=BF, scopes=False, cp=dict(disable_bounds_checks=True, disable_semaphore_checks=True), xfirst=False,
)

def make(**kw):
    cfg = dict(DEF); cfg.update(kw)
    cfg['wout'] = (cfg['w0'], cfg['w1'] or [128] * 8, cfg['w2'] or [128] * cfg['na'])
    NU = cfg['NU']; n3 = cfg['n3']; sub = cfg['sub']; KP = cfg['kp']; KO = [sum(KP[:i]) for i in range(len(KP))]; lag3 = cfg['lag3']; ODT = cfg['odt']
    NA = cfg['na']; NB = NC - n3; subs = {j: (sub if j == NC - 1 else cfg['sub6']) for j in range(n3, NC)}; SM = max(subs.values())
    scope = jax.named_scope if cfg['scopes'] else (lambda n: contextlib.nullcontext())
    nsem_w = sum(len(p) for p in cfg['win']) + sum(len(p) for p in cfg['wout']) + (NC - NA) * len(KP)

    def ds(i, n):
        return pl.ds(i * n if isinstance(i, int) else pl.multiple_of(i * n, n), n)

    def fn(x, wi0, wo0, wi1, wo1, wi2, wo2):
        def body(x_hbm, wi0, wo0, wi1, wo1, wi2, wo2, ob,
                 xs, xg, hb, wib, wob, acc, t1, tr1, t2, tr2, b1, br1, b2, br2,
                 wsem, xsem, xsend, xrecv, tsend, trecv, gsend, grecv, bsend, brecv):
            wis = (wi0, wi1, wi2); wos = (wo0, wo1, wo2)
            xcp = pltpu.make_async_copy(x_hbm, xs, xsem)
            if cfg['xfirst']: xcp.start()
            up_wait = []; dn_wait = []; k = 0
            later = {1: [], 2: [], 3: []}
            def wload(src, dst, sls, k):
                cps = [pltpu.make_async_copy(src.at[sl], dst.at[sl], wsem.at[k]) for sl in sls]
                if src is wos[2]: later[2 if len(later[2]) < 16 else 3].extend(cps)
                elif src is wos[1] or src is wis[2]: later[1].extend(cps)
                else:
                    for c in cps: c.start(priority=1)
                return cps
            halves = [pl.ds(0, 8), pl.ds(8, 8)]
            for l in range(L):
                c0 = 0
                for w in cfg['win'][l]:
                    up_wait.append((l, c0 // NU, wload(wis[l], wib.at[l], [(slice(None), pl.ds(c0, w))], k))); k += 1; c0 += w
                    if k == 1 and not cfg['xfirst']: xcp.start()
                c0 = 0
                for w in cfg['wout'][l]:
                    sls = [(slice(None), r, pl.ds(c0, w)) for r in (halves if w == CW else [slice(None)])]
                    dn_wait.append((l, c0 // CW, 0, wload(wos[l], wob.at[l], sls, k))); k += 1; c0 += w
            for j in range(NA, NC):
                for p, (k0, kk) in enumerate(zip(KO, KP)):
                    sls = [(pl.ds(k0 // 16, kk // 16), r, ds(j, CW)) for r in (halves if cfg['lpar'][p] == 2 else [slice(None)])]
                    dn_wait.append((2, j, p, wload(wos[2], wob.at[2], sls, k))); k += 1

            me = lax.axis_index("i")
            pa = jnp.bitwise_xor(me, 1); pb = 3 - me; pd = jnp.bitwise_xor(me, 2)
            cx = me // 2; cy = jnp.bitwise_and(jnp.bitwise_xor(me, cx), 1)
            bar = pltpu.get_barrier_semaphore()
            for t in (pd, pa, pb):
                pl.semaphore_signal(bar, 1, device_id=(t,), device_id_type=MESH)
            xcp.wait()
            xg[0, ds(me, 64), :] = xs[...].astype(BF)
            pl.semaphore_wait(bar, 3)

            def rcopy(src, dst, ss, rsem, to):
                return pltpu.make_async_remote_copy(src, dst, ss, rsem, device_id=(to,), device_id_type=MESH)
            def wait_all(buf, sem): pltpu.make_async_copy(buf, buf, sem).wait()
            def add(a, b): return a.astype(F32) + b.astype(F32)
            mine = xg.at[0, ds(me, 64)]
            for i, t in enumerate((pd, pa, pb)): rcopy(mine, mine, xsend.at[i], xrecv.at[i], t).start()
            with scope('xag'):
                for i, t in enumerate((pd, pa, pb)): wait_all(xg.at[0, ds(t, 64)], xrecv.at[i])
                for i in range(3): wait_all(mine, xsend.at[i])

            qm = (cy, 2 + cx); qo = (1 - cy, 3 - cx)
            def with_dst(l, f):
                pl.when(l < L - 1)(lambda: f(xg.at[jnp.minimum(l + 1, L - 1)]))
                pl.when(l == L - 1)(lambda: f(ob))

            def up(l):
                def step(n, _):
                    for (ll, nn, cps) in up_wait:
                        @pl.when((l == ll) & (n == nn))
                        def _():
                            with scope('w_up'):
                                for c in cps: c.wait()
                    r = jnp.dot(xg[l], wib[l, :, ds(n, NU)].astype(BF), preferred_element_type=F32)
                    hb[:, ds(n, NU)] = jnp.maximum(r, 0.0).astype(BF)
                lax.fori_loop(0, H // NU, step, None)
            def w_wait(l, j, p, js):
                for (ll, jj, pp, cps) in dn_wait:
                    if pp == p and jj in js:
                        @pl.when((l == ll) & (j == jj))
                        def _():
                            with scope('w_dn'):
                                for c in cps: c.wait()
            def w_val(l, j, k0, kk):
                return wob[l, pl.ds(k0 // 16, kk // 16), :, ds(j, CW)].reshape(kk, CW).astype(BF)

            def t_p1(s, v):
                for q in range(4):
                    keep = (cy == q) if q < 2 else (cx == q - 2)
                    t1[keep.astype(jnp.int32), s, q // 2] = v[q * 64:(q + 1) * 64]
                for h, t in enumerate((pa, pb)):
                    rcopy(t1.at[0, s, h], tr1.at[s, h], tsend.at[0], trecv.at[0, s], t).start()
            def t_p2(s):
                with scope('t2'): wait_all(tr1.at[s], trecv.at[0, s])
                t2[s] = add(t1[1, s], tr1[s]).astype(BF)
                for h, t in enumerate((pb, pa)):
                    rcopy(t2.at[s, h], tr2.at[s, h], tsend.at[1], trecv.at[1, s], t).start()
            def t_p3(l, j):
                s = l * n3 + j
                with scope('t3'): wait_all(tr2.at[s], trecv.at[1, s])
                def f(dst):
                    for h, t in enumerate((pa, pb)):
                        dst[ds(qm[h], 64), ds(j, CW)] = add(t2[s, h], tr2[s, h]).astype(dst.dtype)
                        r = dst.at[ds(qm[h], 64), ds(j, CW)]
                        rcopy(r, r, gsend.at[l, h], grecv.at[l, h], t).start()
                with_dst(l, f)
            def b_p1(l, j, i, v):
                s = l * NB + j - n3; rs = B // (2 * subs[j])
                b1[s, ds(i, 2 * rs)] = v
                for h, t in enumerate((pa, pb)):
                    r = ds(2 * i + h, rs)
                    rcopy(b1.at[s, r], br1.at[s, r], bsend.at[0], brecv.at[0, s, i], t).start()
            def b_p2(l, j):
                s = l * NB + j - n3; rs = B // (2 * subs[j])
                for i in range(subs[j]):
                    rows = ds(i, 2 * rs)
                    with scope('b2'): wait_all(br1.at[s, rows], brecv.at[0, s, i])
                    b2[s, rows] = add(b1[s, rows], br1[s, rows]).astype(BF)
                    for h, t in enumerate((pb, pa)):
                        r = ds(2 * i + h, rs)
                        rcopy(b2.at[s, r], br2.at[s, r], bsend.at[1], brecv.at[1, s, i], t).start()
            def b_fin(l, j):
                s = l * NB + j - n3; rs = B // (2 * subs[j])
                for i in range(subs[j]):
                    rows = ds(i, 2 * rs)
                    with scope('bf'): wait_all(br2.at[s, rows], brecv.at[1, s, i])
                    def f(dst):
                        dst[rows, ds(j, CW)] = add(b2[s, rows], br2[s, rows]).astype(dst.dtype)
                    with_dst(l, f)
            def advance(l, j):
                pl.when((j >= 1) & (j - 1 < n3))(lambda: t_p2(l * n3 + j - 1))
                pl.when((j >= lag3) & (j - lag3 < n3))(lambda: t_p3(l, j - lag3))

            def layer(l, _):
                for ll in (1, 2):
                    @pl.when(l == ll)
                    def _():
                        for c in later[ll]: c.start(priority=1)
                with scope('up'): up(l)
                def step_a(j, _):
                    @pl.when((l == 2) & (j == 2))
                    def _():
                        for c in later[3]: c.start(priority=1)
                    w_wait(l, j, 0, range(NA))
                    with scope('mm'):
                        v = jnp.dot(hb[...], w_val(l, j, 0, H), preferred_element_type=F32).astype(BF)
                    t_p1(l * n3 + j, v)
                    advance(l, j)
                lax.fori_loop(0, NA, step_a, None)
                def gwait(dst):
                    for h in range(2):
                        wait_all(dst.at[ds(qo[h], 64), pl.ds(0, n3 * CW)], grecv.at[l, h])
                        wait_all(dst.at[ds(qm[h], 64), pl.ds(0, n3 * CW)], gsend.at[l, h])
                for op in cfg['tail'].split():
                    c, j = op[:-1], int(op[-1])
                    if c in 'abc':
                        p = 'abc'.index(c); k0, kk = KO[p], KP[p]
                        w_wait(l, j, p, (j,))
                        if p < len(KP) - 1:
                            with scope('mma'):
                                r = jnp.dot(hb[:, pl.ds(k0, kk)], w_val(l, j, k0, kk), preferred_element_type=F32)
                                acc[...] = r if p == 0 else acc[...] + r
                        else:
                            with scope('mmb'):
                                w = w_val(l, j, k0, kk)
                                if j < n3:
                                    t_p1(l * n3 + j, (acc[...] + jnp.dot(hb[:, pl.ds(k0, kk)], w, preferred_element_type=F32)).astype(BF))
                                else:
                                    for i in range(subs[j]):
                                        rows = ds(i, B // subs[j])
                                        v = acc[rows, :] + jnp.dot(hb[rows, pl.ds(k0, kk)], w, preferred_element_type=F32)
                                        b_p1(l, j, i, v.astype(BF))
                    elif c == 's': (t_p2(l * n3 + j) if j < n3 else b_p2(l, j))
                    elif c == 't': (t_p3(l, j) if j < n3 else b_fin(l, j))
                    elif c == 'g':
                        with scope('gw'): with_dst(l, gwait)
                        wait_all(t1.at[0, pl.ds(l * n3, n3)], tsend.at[0])
                        wait_all(t2.at[pl.ds(l * n3, n3)], tsend.at[1])
                        wait_all(b1.at[pl.ds(l * NB, NB)], bsend.at[0])
                wait_all(b2.at[pl.ds(l * NB, NB)], bsend.at[1])
            lax.fori_loop(0, L, layer, None)

        DMA = pltpu.SemaphoreType.DMA
        tp = pltpu.VMEM((L * n3, 2, 64, CW), BF); bp = pltpu.VMEM((L * NB, B, CW), BF)
        return pl.pallas_call(
            body, out_shape=jax.ShapeDtypeStruct((B, D), ODT),
            in_specs=[pl.BlockSpec(memory_space=pltpu.HBM)] * 7,
            out_specs=pl.BlockSpec(memory_space=pltpu.VMEM),
            scratch_shapes=[
                pltpu.VMEM((64, D), F32), pltpu.VMEM((L, B, D), BF), pltpu.VMEM((B, H), BF),
                pltpu.VMEM((L, D, H), F32), pltpu.VMEM((L, H // 16, 16, D), F32), pltpu.VMEM((B, CW), F32),
                pltpu.VMEM((2, L * n3, 2, 64, CW), BF), tp, tp, tp, bp, bp, bp, bp,
                DMA((nsem_w,)), DMA, DMA((3,)), DMA((3,)), DMA((2,)), DMA((2, L * n3)), DMA((L, 2)), DMA((L, 2)),
                DMA((2,)), DMA((2, L * NB, SM)),
            ],
            compiler_params=pltpu.CompilerParams(collective_id=0, vmem_limit_bytes=100 * 2**20, **cfg['cp']),
        )(x, wi0, wo0.reshape(H // 16, 16, D), wi1, wo1.reshape(H // 16, 16, D), wi2, wo2.reshape(H // 16, 16, D))
    return fn


def pallas_dist_mlpseq_tp1d_bs_rep_b64_d1024_h2048_kernel(x, Win0, Wout0, Win1, Wout1, Win2, Wout2):
    return make(**dict(sub=4))(x, Win0, Wout0, Win1, Wout1, Win2, Wout2)
```

```python
import jax
import jax.numpy as jnp
from jax import lax
from jax.experimental import pallas as pl
from jax.experimental.pallas import tpu as pltpu

BF16 = jnp.bfloat16
F32 = jnp.float32

B, D, H, L = 256, 1024, 2048, 3
XR = B // 4
CW = 128
NC = D // CW
NU = 512
NBLK = H // NU
KU = D // 2
IR = 64
OR = 32
N_LO = 4
N_LOOP = 5
QUEUE = 25

WIN_PIECES = (
    ((2048,), (2048,)),
    ((1024, 1024), (1024, 1024)),
    ((1024, 1024), (1024, 1024)),
)
LENT = (
    (1, "a", (("x", 9), (("up", 0, 1), 2), (("up", 0, 3), 2), (("up", 0, 5), 2),
              (("down", 0, 4), 1))),
    (2, "b", (("entry", 3), (("up", 0, 2), 1), (("up", 0, 4), 1), (("up", 0, 6), 1),
              (("up", 0, 7), 1), (("down", 0, 1), 1), (("up", 1, 0), 1), (("up", 1, 2), 1),
              (("up", 1, 4), 1), (("up", 1, 6), 1), (("down", 1, 1), 1), (("down", 1, 3), 1),
              (("up", 2, 0), 2))),
    (2, "a", (("fwd", 2), (("up", 0, 7), 2), (("up", 1, 0), 3), (("up", 1, 2), 2),
              (("up", 1, 3), 1), (("up", 1, 6), 1), (("up", 1, 7), 1), (("down", 1, 2), 1),
              (("down", 1, 4), 1), (("up", 2, 0), 2))),
)
RELAY_WOUT1, RELAY_WIN2 = 8, 6
RELAY_WOUT2 = (
    (3, 0, ("up", 2, 6), ("down", 2, 0), ("down", 2, 3)),
    (3, 1, ("up", 2, 7), ("down", 2, 1), ("down", 2, 3)),
    (4, 0, ("down", 2, 2), ("down", 2, 3), ("down", 2, 4)),
)
N_SLOTS = tuple(sum(1 for s in LENT if s[0] == l) for l in range(L))
N_LENT_COPIES = sum(len(s[2]) for s in LENT)
N_PIECES = sum(len(h) for w in WIN_PIECES for h in w) + L * NC + (NC - N_LOOP)
N_RELAY = RELAY_WOUT1 + RELAY_WIN2 + len(RELAY_WOUT2)


def _ds(i, n):
    return pl.ds(i * n if isinstance(i, int) else pl.multiple_of(i * n, n), n)


def _wait_all(buf, sem):
    pltpu.make_async_copy(buf, buf, sem).wait()


def _add(a, b):
    return (a.astype(F32) + b.astype(F32)).astype(BF16)


def _body(
    x_hbm, wi0, wo0, wi1, wo1, wi2, wo2, out,
    xs, xg, hb, h_back, wib, wob, acc_dn, acc_up,
    t1, t1_in, t2, t2_in, b1, b1_in, b2, b2_in, relay_rows, relay_tiles,
    w_sem, relay_sem, x_sem, x_send, x_recv, lent_send, lent_recv, h_send, h_recv,
    p_send, p_recv, g_send, g_recv,
):
    wis, wos = (wi0, wi1, wi2), (wo0, wo1, wo2)

    waits, starts = {}, {}

    def on(table, when, action):
        table.setdefault(when, []).append(action)

    def start_local(copy):
        return lambda: copy.start(priority=1)

    def run(when):
        for action in waits.get(when, []) + starts.get(when, []):
            action()

    def run_at(kind, l, n, candidates):
        for ll in range(L):
            todo = [nn for nn in candidates if (kind, ll, nn) in waits or (kind, ll, nn) in starts]
            if todo:

                @pl.when(l == ll)
                def _():
                    for nn in todo:
                        if isinstance(n, int):
                            run((kind, ll, nn))
                        else:
                            pl.when(n == nn)(lambda: run((kind, ll, nn)))

    stream, top_up, sem_ids = [], [("start", 0), ("gathered", 8)], iter(range(N_PIECES))

    def piece(src, dst, slices, when):
        sem = w_sem.at[next(sem_ids)]
        for sl in slices:
            copy = pltpu.make_async_copy(src.at[sl], dst.at[sl], sem)
            stream.append(copy)
            on(waits, when, copy.wait)
        top_up.append((when, len(stream)))

    for l in range(L):
        for kh in range(2):
            c0 = 0
            for width in WIN_PIECES[l][kh]:
                slices = []
                for c in range(c0, c0 + width, H // 2):
                    first = max(c, CW * N_SLOTS[l])
                    for i in range(IR // 8):
                        relayed = int((l, kh, c) == (2, 1, H // 2) and i < RELAY_WIN2)
                        groups = pl.ds(kh * KU // IR, KU // IR - relayed)
                        slices.append((groups, _ds(i, 8), pl.ds(first, c + H // 2 - first)))
                piece(wis[l], wib.at[l], slices, ("up", l, kh * NBLK + c0 // NU))
                c0 += width
        for j in range(NC):
            parts = 2 if l == L - 1 and j >= N_LOOP else 1
            for p in range(parts):
                slices = []
                for i in range(OR // 8):
                    relayed = len(range(i, RELAY_WOUT1, OR // 8)) if l == 1 else 0
                    relayed += 8 * sum(1 for r in RELAY_WOUT2 if (l, r[0], r[1], p) == (2, j, i, parts - 1))
                    n = H // OR // parts
                    slices.append((pl.ds(p * n, n - relayed), _ds(i, 8), _ds(j, CW)))
                piece(wos[l], wob.at[l], slices, ("late" if p else "down", l, j))
        if l < L - 1:
            top_up.append((("tail", l, 0), len(stream) + 12))
    issued = 0
    for when, landed in top_up:
        assert when not in waits or landed <= issued
        for copy in stream[issued:landed + QUEUE]:
            on(starts, when, start_local(copy))
        issued = max(issued, min(landed + QUEUE, len(stream)))

    run("start")
    x_copy = pltpu.make_async_copy(x_hbm, xs, x_sem)
    x_copy.start()

    me = lax.axis_index("i")
    pa = jnp.bitwise_xor(me, 1)
    pb = 3 - me
    pd = jnp.bitwise_xor(me, 2)
    cb = me // 2
    ca = jnp.bitwise_and(jnp.bitwise_xor(me, cb), 1)

    def remote(src, dst, send_sem, recv_sem, to):
        return pltpu.make_async_remote_copy(
            src, dst, send_sem, recv_sem, device_id=(to,), device_id_type=pl.DeviceIdType.MESH
        )

    returns, k = [], 0
    for i, (l, link, parts) in enumerate(LENT):
        to = pa if link == "a" else pb
        slot = sum(1 for s in LENT[:i] if s[0] == l)
        g = 0
        for when, n in parts:
            sl = (pl.ds(g, n), slice(None), _ds(slot, CW))
            copy = remote(wis[l].at[sl], wib.at[l].at[sl], lent_send.at[k], lent_recv.at[k], to)
            on(starts, when, copy.start)
            on(waits, ("up", l, 0 if g * IR < KU else NBLK), copy.wait)
            g, k = g + n, k + 1
        assert g * IR == D
        back = remote(hb.at[slot], h_back.at[i], h_send.at[i], h_recv.at[i], to)
        on(starts, ("up", l, NBLK + 1), back.start)
        returns.append((l, i, slot, back))

    relays = []
    for i in range(RELAY_WOUT1):
        sl = (H // OR - 1 - i // (OR // 8), _ds(i % (OR // 8), 8))
        relays.append((wo1.at[sl], relay_rows.at[i], wob.at[1].at[sl],
                       ("down", 0, i), ("up", 1, i), ("down", 1, 0)))
    for i in range(RELAY_WIN2):
        sl = (D // IR - 1, _ds(i, 8), pl.ds(H // 2, H // 2))
        relays.append((wi2.at[sl], relay_rows.at[i], wib.at[2].at[sl],
                       ("down", 1, i), ("up", 2, i), ("up", 2, NBLK + NBLK // 2)))
    for i, (j, phase, load_at, forward_at, needed_at) in enumerate(RELAY_WOUT2):
        sl = (pl.ds(H // OR - 8, 8), _ds(phase, 8), _ds(j, CW))
        relays.append((wo2.at[sl], relay_tiles.at[i], wob.at[2].at[sl],
                       load_at, forward_at, needed_at))
    for i, (src, via, dst, load_at, forward_at, needed_at) in enumerate(relays):
        load = pltpu.make_async_copy(src, via, relay_sem.at[0, i])
        forward = pltpu.make_async_copy(via, dst, relay_sem.at[1, i])
        on(starts, load_at, start_local(load))
        on(waits, forward_at, load.wait)
        on(starts, forward_at, start_local(forward))
        on(waits, needed_at, forward.wait)

    barrier = pltpu.get_barrier_semaphore()
    for to in (pa, pb):
        pl.semaphore_signal(barrier, 1, device_id=(to,), device_id_type=pl.DeviceIdType.MESH)
    pl.semaphore_wait(barrier, 2)
    run("entry")

    def x_rows(chip):
        return xg.at[0, :, _ds(chip, XR)]

    x_copy.wait()
    for j in range(NC):
        xg[0, j, _ds(me, XR)] = xs[:, _ds(j, CW)].astype(BF16)
    remote(x_rows(me), x_rows(me), x_send.at[0], x_recv.at[0], pa).start()
    remote(x_rows(me), x_rows(me), x_send.at[1], x_recv.at[1], pb).start()
    run("x")
    _wait_all(x_rows(pa), x_recv.at[0])
    remote(x_rows(pa), x_rows(pa), x_send.at[2], x_recv.at[2], pb).start()
    run("fwd")
    run("gathered")
    _wait_all(x_rows(pb), x_recv.at[1])
    _wait_all(x_rows(pd), x_recv.at[2])
    _wait_all(x_rows(me), x_send.at[0])
    _wait_all(x_rows(me), x_send.at[1])
    _wait_all(x_rows(pa), x_send.at[2])

    def result(dst, rows, j, n=None):
        if dst is out:
            return dst.at[rows, _ds(j, CW) if n is None else pl.ds(j * CW, n * CW)]
        return dst.at[j if n is None else pl.ds(j, n), rows]

    mine = (ca, 2 + cb)
    theirs = (1 - ca, 3 - cb)

    def three_1(s, v, grp):
        for q in range(4):
            t1[(mine[q // 2] == q).astype(jnp.int32), s, q // 2] = v[q * XR:(q + 1) * XR]
        for h, to in enumerate((pa, pb)):
            remote(t1.at[0, s, h], t1_in.at[s, h], p_send.at[grp, 0], p_recv.at[0, s, 0], to).start()

    def three_2(s, grp):
        _wait_all(t1_in.at[s], p_recv.at[0, s, 0])
        t2[s] = _add(t1[1, s], t1_in[s])
        for h, to in enumerate((pb, pa)):
            remote(t2.at[s, h], t2_in.at[s, h], p_send.at[grp, 1], p_recv.at[1, s, 0], to).start()

    def three_3(l, j, grp):
        s = l * NC + j
        _wait_all(t2_in.at[s], p_recv.at[1, s, 0])

        def finish(dst):
            for h, to in enumerate((pa, pb)):
                r = result(dst, _ds(mine[h], XR), j)
                r[...] = _add(t2[s, h], t2_in[s, h])
                remote(r, r, g_send.at[l, grp, h], g_recv.at[l, grp, h], to).start()

        pl.when(l < L - 1)(lambda: finish(xg.at[jnp.minimum(l + 1, L - 1)]))
        pl.when(l == L - 1)(lambda: finish(out))

    def three_done(l, j, n, grp, dst):
        for h in range(2):
            _wait_all(result(dst, _ds(theirs[h], XR), j, n), g_recv.at[l, grp, h])
            _wait_all(result(dst, _ds(mine[h], XR), j, n), g_send.at[l, grp, h])
        _wait_all(t1.at[0, pl.ds(l * NC + j, n)], p_send.at[grp, 0])
        _wait_all(t2.at[pl.ds(l * NC + j, n)], p_send.at[grp, 1])

    def fly_send(src, dst, phase, s, i, n, grp):
        for h, to in enumerate((pa, pb) if phase == 0 else (pb, pa)):
            r = _ds(2 * i + h, n // 2)
            remote(src.at[s, r], dst.at[s, r], p_send.at[grp, phase], p_recv.at[phase, s, i], to).start()

    def fly_1(s, i, n, v, grp):
        b1[s, _ds(i, n)] = v
        fly_send(b1, b1_in, 0, s, i, n, grp)

    def fly_2(s, i, n, grp):
        _wait_all(b1_in.at[s, _ds(i, n)], p_recv.at[0, s, i])
        b2[s, _ds(i, n)] = _add(b1[s, _ds(i, n)], b1_in[s, _ds(i, n)])
        fly_send(b2, b2_in, 1, s, i, n, grp)

    def fly_done(l, j, i, n, dst):
        s = l * NC + j
        _wait_all(b2_in.at[s, _ds(i, n)], p_recv.at[1, s, i])
        result(dst, _ds(i, n), j)[...] = _add(b2[s, _ds(i, n)], b2_in[s, _ds(i, n)])

    def finish_upper(l, dst):
        last_two = pl.ds(l * NC + NC - 2, 2)
        _wait_all(b1.at[last_two], p_send.at[2, 0])
        three_done(l, N_LO, 2, 1, dst)
        for j in (NC - 2, NC - 1):
            for i in range(2):
                fly_done(l, j, i, B // 2, dst)
        _wait_all(b2.at[last_two], p_send.at[2, 1])

    def down(l, j, k0, kk, w=None, rows=slice(None)):
        h = jnp.concatenate([hb[i, rows] for i in range(k0 // CW, (k0 + kk) // CW)], axis=1)
        return jnp.dot(h, wout(l, j, k0, kk) if w is None else w, preferred_element_type=F32)

    def wout(l, j, k0, kk):
        return wob[l, pl.ds(k0 // OR, kk // OR), :, _ds(j, CW)].reshape(kk, CW).astype(BF16)

    def layer(l, _):
        inner = l < L - 1
        pl.when(l > 0)(lambda: three_done(l - 1, 0, N_LO, 0, xg.at[l]))

        def up_step(n, _):
            pl.when((l > 0) & (n == NBLK))(lambda: finish_upper(l - 1, xg.at[l]))
            run_at("up", l, n, range(2 * NBLK))
            kh, blk = n // NBLK, n % NBLK
            xk = jnp.concatenate([xg[l, kh * N_LO + i] for i in range(N_LO)], axis=1)
            w = wib[l, _ds(kh, KU // IR), :, _ds(blk, NU)].reshape(KU, NU).astype(BF16)
            r = jnp.dot(xk, w, preferred_element_type=F32) + jnp.where(kh == 1, acc_up[blk], 0.0)
            acc_up[blk] = r
            h = jnp.maximum(r, 0.0).astype(BF16)
            for i in range(NU // CW):
                hb[blk * (NU // CW) + i] = h[:, i * CW:(i + 1) * CW]

        lax.fori_loop(0, 2 * NBLK, up_step, None)
        for ll, i, slot, back in returns:

            @pl.when(l == ll)
            def _():
                back.wait()
                hb[slot] = h_back[i]

        def down_step(j, _):
            s = l * NC + j
            run_at("down", l, j, range(N_LOOP))
            v = down(l, j, 0, H).astype(BF16)
            pl.when(j >= N_LO)(lambda: three_1(s, v, 1))

            @pl.when(inner)
            def _():
                pl.when(j < N_LO)(lambda: three_1(s, v, 0))
                pl.when(j >= 1)(lambda: three_2(s - 1, 0))
                pl.when(j >= 3)(lambda: three_3(l, j - 3, 0))

            @pl.when(jnp.logical_not(inner))
            def _():
                pl.when(j < N_LO)(lambda: fly_1(s, 0, B, v, 0))
                pl.when(j >= 2)(lambda: fly_2(s - 2, 0, B, 0))

        lax.fori_loop(0, N_LOOP, down_step, None)

        s0, half = l * NC, H // 2

        def first_half(j):
            run_at("down", l, j, (j,))
            acc_dn[...] = down(l, j, 0, half)

        first_half(5)
        pl.when(inner)(lambda: three_3(l, 2, 0))
        run_at("late", l, 5, (5,))
        three_1(s0 + 5, (acc_dn[...] + down(l, 5, half, half)).astype(BF16), 1)
        pl.when(jnp.logical_not(inner))(lambda: fly_2(s0 + 3, 0, B, 0))

        first_half(6)
        pl.when(inner)(lambda: three_3(l, 3, 0))
        three_2(s0 + 4, 1)
        run_at("late", l, 6, (6,))
        v = (acc_dn[...] + down(l, 6, half, half)).astype(BF16)
        for i in range(2):
            fly_1(s0 + 6, i, B // 2, v[i * B // 2:(i + 1) * B // 2], 2)

        first_half(7)
        three_2(s0 + 5, 1)
        run_at("late", l, 7, (7,))
        w = wout(l, 7, half, half)
        for i in range(2):
            rows = _ds(i, B // 2)
            fly_1(s0 + 7, i, B // 2, (acc_dn[rows] + down(l, 7, half, half, w, rows)).astype(BF16), 2)

        three_3(l, 4, 1)
        for i in range(2):
            fly_2(s0 + 6, i, B // 2, 2)
        three_3(l, 5, 1)
        run_at("tail", l, 0, (0,))
        for i in range(2):
            fly_2(s0 + 7, i, B // 2, 2)

    lax.fori_loop(0, L, layer, None)

    lower = pl.ds((L - 1) * NC, N_LO)
    lax.fori_loop(0, N_LO, lambda j, _: fly_done(L - 1, j, 0, B, out), None)
    _wait_all(b1.at[lower], p_send.at[0, 0])
    _wait_all(b2.at[lower], p_send.at[0, 1])
    finish_upper(L - 1, out)


def pallas_dist_mlpseq_tp1d_bs_rep_b64_d1024_h2048_kernel(
    x: jax.Array,
    Win0: jax.Array,
    Wout0: jax.Array,
    Win1: jax.Array,
    Wout1: jax.Array,
    Win2: jax.Array,
    Wout2: jax.Array,
):
    dma = pltpu.SemaphoreType.DMA
    quarters = pltpu.VMEM((L * NC, 2, XR, CW), BF16)
    chunks = pltpu.VMEM((L * NC, B, CW), BF16)
    win_view, wout_view = (D // IR, IR, H), (H // OR, OR, D)
    return pl.pallas_call(
        _body,
        out_shape=jax.ShapeDtypeStruct((B, D), BF16),
        in_specs=[pl.BlockSpec(memory_space=pltpu.HBM)] * 7,
        out_specs=pl.BlockSpec(memory_space=pltpu.VMEM),
        scratch_shapes=[
            pltpu.VMEM((XR, D), F32),
            pltpu.VMEM((L, NC, B, CW), BF16),
            pltpu.VMEM((H // CW, B, CW), BF16),
            pltpu.VMEM((len(LENT), B, CW), BF16),
            pltpu.VMEM((L, *win_view), F32),
            pltpu.VMEM((L, *wout_view), F32),
            pltpu.VMEM((B, CW), F32),
            pltpu.VMEM((NBLK, B, NU), F32),
            pltpu.VMEM((2, L * NC, 2, XR, CW), BF16),
            quarters, quarters, quarters,
            chunks, chunks, chunks, chunks,
            pltpu.SMEM((max(RELAY_WOUT1, RELAY_WIN2), 8, D), F32),
            pltpu.SMEM((len(RELAY_WOUT2), 8, 8, CW), F32),
            dma((N_PIECES,)), dma((2, N_RELAY)), dma, dma((3,)), dma((3,)),
            dma((N_LENT_COPIES,)), dma((N_LENT_COPIES,)), dma((len(LENT),)), dma((len(LENT),)),
            dma((3, 2)), dma((2, L * NC, 2)), dma((L, 2, 2)), dma((L, 2, 2)),
        ],
        compiler_params=pltpu.CompilerParams(
            collective_id=0,
            vmem_limit_bytes=100 * 2**20,
            disable_bounds_checks=True,
        ),
    )(
        x,
        Win0.reshape(win_view), Wout0.reshape(wout_view),
        Win1.reshape(win_view), Wout1.reshape(wout_view),
        Win2.reshape(win_view), Wout2.reshape(wout_view),
    )
```

```python
import jax
import jax.numpy as jnp
from jax import lax
from jax.experimental import pallas as pl
from jax.experimental.pallas import tpu as pltpu

BF16 = jnp.bfloat16
F32 = jnp.float32

B, D, H, L = 256, 1024, 2048, 3
XR = B // 4
CW = 128
NC = D // CW
NU = 512
NBLK = H // NU
KU = D // 2
IR = 64
OR = 32
N_LO = 4
N_LOOP = 5
QUEUE = 25

WIN_PIECES = (
    ((2048,), (2048,)),
    ((1024, 1024), (1024, 1024)),
    ((1024, 1024), (1024, 1024)),
)
LENT = (
    (1, "a", (("x", 9), (("up", 0, 1), 2), (("up", 0, 3), 2), (("up", 0, 5), 2),
              (("down", 0, 4), 1))),
    (2, "b", (("entry", 3), (("up", 0, 2), 1), (("up", 0, 6), 1), (("up", 0, 7), 1),
              (("down", 0, 1), 1), (("down", 0, 3), 1), (("up", 1, 0), 1), (("up", 1, 2), 1),
              (("up", 1, 6), 1), (("down", 1, 1), 1), (("down", 1, 3), 1), (("tail", 1, 0), 1),
              (("up", 2, 0), 2))),
    (2, "a", (("fwd", 2), (("up", 0, 7), 2), (("up", 1, 0), 3), (("up", 1, 2), 1),
              (("up", 1, 3), 1), (("up", 1, 6), 1), (("up", 1, 7), 1), (("down", 1, 0), 1),
              (("down", 1, 2), 1), (("down", 1, 4), 1), (("up", 2, 0), 2))),
)
RELAY_WOUT1, RELAY_WIN2 = 8, 6
RELAY_WOUT2 = (
    (3, 0, ("up", 2, 6), ("down", 2, 0), ("down", 2, 3)),
    (3, 1, ("up", 2, 7), ("down", 2, 1), ("down", 2, 3)),
    (4, 0, ("down", 2, 2), ("down", 2, 3), ("down", 2, 4)),
)
N_SLOTS = tuple(sum(1 for s in LENT if s[0] == l) for l in range(L))
N_LENT_COPIES = sum(len(s[2]) for s in LENT)
N_PIECES = sum(len(h) for w in WIN_PIECES for h in w) + L * NC + (NC - N_LOOP)
N_RELAY = RELAY_WOUT1 + RELAY_WIN2 + len(RELAY_WOUT2)


def _ds(i, n):
    return pl.ds(i * n if isinstance(i, int) else pl.multiple_of(i * n, n), n)


def _wait_all(buf, sem):
    pltpu.make_async_copy(buf, buf, sem).wait()


def _add(a, b):
    return (a.astype(F32) + b.astype(F32)).astype(BF16)


def _body(
    x_hbm, wi0, wo0, wi1, wo1, wi2, wo2, out,
    xs, xg, hb, h_back, wib, wob, acc_dn, acc_up,
    t1, t1_in, t2, t2_in, b1, b1_in, b2, b2_in, relay_rows, relay_tiles,
    w_sem, relay_sem, x_sem, x_send, x_recv, lent_send, lent_recv, h_send, h_recv,
    p_send, p_recv, g_send, g_recv,
):
    wis, wos = (wi0, wi1, wi2), (wo0, wo1, wo2)

    waits, starts = {}, {}

    def on(table, when, action):
        table.setdefault(when, []).append(action)

    def start_local(copy):
        return lambda: copy.start(priority=1)

    def run(when):
        for action in waits.get(when, []) + starts.get(when, []):
            action()

    def run_at(kind, l, n, candidates):
        for ll in range(L):
            todo = [nn for nn in candidates if (kind, ll, nn) in waits or (kind, ll, nn) in starts]
            if todo:

                @pl.when(l == ll)
                def _():
                    for nn in todo:
                        if isinstance(n, int):
                            run((kind, ll, nn))
                        else:
                            pl.when(n == nn)(lambda: run((kind, ll, nn)))

    stream, top_up, sem_ids = [], [("start", 0), ("gathered", 8)], iter(range(N_PIECES))

    def piece(src, dst, slices, when):
        sem = w_sem.at[next(sem_ids)]
        for sl in slices:
            copy = pltpu.make_async_copy(src.at[sl], dst.at[sl], sem)
            stream.append(copy)
            on(waits, when, copy.wait)
        top_up.append((when, len(stream)))

    for l in range(L):
        for kh in range(2):
            c0 = 0
            for width in WIN_PIECES[l][kh]:
                slices = []
                for c in range(c0, c0 + width, H // 2):
                    first = max(c, CW * N_SLOTS[l])
                    for i in range(IR // 8):
                        relayed = int((l, kh, c) == (2, 1, H // 2) and i < RELAY_WIN2)
                        groups = pl.ds(kh * KU // IR, KU // IR - relayed)
                        slices.append((groups, _ds(i, 8), pl.ds(first, c + H // 2 - first)))
                piece(wis[l], wib.at[l], slices, ("up", l, kh * NBLK + c0 // NU))
                c0 += width
        for j in range(NC):
            parts = 2 if l == L - 1 and j >= N_LOOP else 1
            for p in range(parts):
                slices = []
                for i in range(OR // 8):
                    relayed = len(range(i, RELAY_WOUT1, OR // 8)) if l == 1 else 0
                    relayed += 8 * sum(1 for r in RELAY_WOUT2 if (l, r[0], r[1], p) == (2, j, i, parts - 1))
                    n = H // OR // parts
                    slices.append((pl.ds(p * n, n - relayed), _ds(i, 8), _ds(j, CW)))
                piece(wos[l], wob.at[l], slices, ("late" if p else "down", l, j))
        if l < L - 1:
            top_up.append((("late", l, NC - 1), len(stream) + 6))
            top_up.append((("tail", l, 0), len(stream) + 12))
    issued = 0
    for when, landed in top_up:
        assert when not in waits or landed <= issued
        for copy in stream[issued:landed + QUEUE]:
            on(starts, when, start_local(copy))
        issued = max(issued, min(landed + QUEUE, len(stream)))

    run("start")
    x_copy = pltpu.make_async_copy(x_hbm, xs, x_sem)
    x_copy.start()

    me = lax.axis_index("i")
    pa = jnp.bitwise_xor(me, 1)
    pb = 3 - me
    pd = jnp.bitwise_xor(me, 2)
    cb = me // 2
    ca = jnp.bitwise_and(jnp.bitwise_xor(me, cb), 1)

    def remote(src, dst, send_sem, recv_sem, to):
        return pltpu.make_async_remote_copy(
            src, dst, send_sem, recv_sem, device_id=(to,), device_id_type=pl.DeviceIdType.MESH
        )

    returns, k = [], 0
    for i, (l, link, parts) in enumerate(LENT):
        to = pa if link == "a" else pb
        slot = sum(1 for s in LENT[:i] if s[0] == l)
        g = 0
        for when, n in parts:
            sl = (pl.ds(g, n), slice(None), _ds(slot, CW))
            copy = remote(wis[l].at[sl], wib.at[l].at[sl], lent_send.at[k], lent_recv.at[k], to)
            on(starts, when, copy.start)
            on(waits, ("up", l, 0 if g * IR < KU else NBLK), copy.wait)
            g, k = g + n, k + 1
        assert g * IR == D
        back = remote(hb.at[slot], h_back.at[i], h_send.at[i], h_recv.at[i], to)
        on(starts, ("up", l, NBLK + 1), back.start)
        returns.append((l, i, slot, back))

    relays = []
    for i in range(RELAY_WOUT1):
        sl = (H // OR - 1 - i // (OR // 8), _ds(i % (OR // 8), 8))
        relays.append((wo1.at[sl], relay_rows.at[i], wob.at[1].at[sl],
                       ("down", 0, i), ("up", 1, i), ("down", 1, 0)))
    for i in range(RELAY_WIN2):
        sl = (D // IR - 1, _ds(i, 8), pl.ds(H // 2, H // 2))
        relays.append((wi2.at[sl], relay_rows.at[i], wib.at[2].at[sl],
                       ("down", 1, i), ("up", 2, i), ("up", 2, NBLK + NBLK // 2)))
    for i, (j, phase, load_at, forward_at, needed_at) in enumerate(RELAY_WOUT2):
        sl = (pl.ds(H // OR - 8, 8), _ds(phase, 8), _ds(j, CW))
        relays.append((wo2.at[sl], relay_tiles.at[i], wob.at[2].at[sl],
                       load_at, forward_at, needed_at))
    for i, (src, via, dst, load_at, forward_at, needed_at) in enumerate(relays):
        load = pltpu.make_async_copy(src, via, relay_sem.at[0, i])
        forward = pltpu.make_async_copy(via, dst, relay_sem.at[1, i])
        on(starts, load_at, start_local(load))
        on(waits, forward_at, load.wait)
        on(starts, forward_at, start_local(forward))
        on(waits, needed_at, forward.wait)

    barrier = pltpu.get_barrier_semaphore()
    for to in (pa, pb):
        pl.semaphore_signal(barrier, 1, device_id=(to,), device_id_type=pl.DeviceIdType.MESH)
    pl.semaphore_wait(barrier, 2)
    run("entry")

    def x_rows(chip):
        return xg.at[0, :, _ds(chip, XR)]

    x_copy.wait()
    for j in range(NC):
        xg[0, j, _ds(me, XR)] = xs[:, _ds(j, CW)].astype(BF16)
    remote(x_rows(me), x_rows(me), x_send.at[0], x_recv.at[0], pa).start()
    remote(x_rows(me), x_rows(me), x_send.at[1], x_recv.at[1], pb).start()
    run("x")
    _wait_all(x_rows(pa), x_recv.at[0])
    remote(x_rows(pa), x_rows(pa), x_send.at[2], x_recv.at[2], pb).start()
    run("fwd")
    run("gathered")
    _wait_all(x_rows(pb), x_recv.at[1])
    _wait_all(x_rows(pd), x_recv.at[2])
    _wait_all(x_rows(me), x_send.at[0])
    _wait_all(x_rows(me), x_send.at[1])
    _wait_all(x_rows(pa), x_send.at[2])

    def result(dst, rows, j, n=None):
        if dst is out:
            return dst.at[rows, _ds(j, CW) if n is None else pl.ds(j * CW, n * CW)]
        return dst.at[j if n is None else pl.ds(j, n), rows]

    mine = (ca, 2 + cb)
    theirs = (1 - ca, 3 - cb)

    def three_1(s, v, grp):
        for q in range(4):
            t1[(mine[q // 2] == q).astype(jnp.int32), s, q // 2] = v[q * XR:(q + 1) * XR]
        for h, to in enumerate((pa, pb)):
            remote(t1.at[0, s, h], t1_in.at[s, h], p_send.at[grp, 0], p_recv.at[0, s, 0], to).start()

    def three_2(s, grp):
        _wait_all(t1_in.at[s], p_recv.at[0, s, 0])
        t2[s] = _add(t1[1, s], t1_in[s])
        for h, to in enumerate((pb, pa)):
            remote(t2.at[s, h], t2_in.at[s, h], p_send.at[grp, 1], p_recv.at[1, s, 0], to).start()

    def three_3(l, j, grp):
        s = l * NC + j
        _wait_all(t2_in.at[s], p_recv.at[1, s, 0])

        def finish(dst):
            for h, to in enumerate((pa, pb)):
                r = result(dst, _ds(mine[h], XR), j)
                r[...] = _add(t2[s, h], t2_in[s, h])
                remote(r, r, g_send.at[l, grp, h], g_recv.at[l, grp, h], to).start()

        pl.when(l < L - 1)(lambda: finish(xg.at[jnp.minimum(l + 1, L - 1)]))
        pl.when(l == L - 1)(lambda: finish(out))

    def three_done(l, j, n, grp, dst):
        for h in range(2):
            _wait_all(result(dst, _ds(theirs[h], XR), j, n), g_recv.at[l, grp, h])
            _wait_all(result(dst, _ds(mine[h], XR), j, n), g_send.at[l, grp, h])
        _wait_all(t1.at[0, pl.ds(l * NC + j, n)], p_send.at[grp, 0])
        _wait_all(t2.at[pl.ds(l * NC + j, n)], p_send.at[grp, 1])

    def fly_send(src, dst, phase, s, i, n, grp):
        for h, to in enumerate((pa, pb) if phase == 0 else (pb, pa)):
            r = _ds(2 * i + h, n // 2)
            remote(src.at[s, r], dst.at[s, r], p_send.at[grp, phase], p_recv.at[phase, s, i], to).start()

    def fly_1(s, i, n, v, grp):
        b1[s, _ds(i, n)] = v
        fly_send(b1, b1_in, 0, s, i, n, grp)

    def fly_2(s, i, n, grp):
        _wait_all(b1_in.at[s, _ds(i, n)], p_recv.at[0, s, i])
        b2[s, _ds(i, n)] = _add(b1[s, _ds(i, n)], b1_in[s, _ds(i, n)])
        fly_send(b2, b2_in, 1, s, i, n, grp)

    def fly_done(l, j, i, n, dst):
        s = l * NC + j
        _wait_all(b2_in.at[s, _ds(i, n)], p_recv.at[1, s, i])
        result(dst, _ds(i, n), j)[...] = _add(b2[s, _ds(i, n)], b2_in[s, _ds(i, n)])

    def finish_upper(l, dst):
        last_two = pl.ds(l * NC + NC - 2, 2)
        _wait_all(b1.at[last_two], p_send.at[2, 0])
        three_done(l, N_LO, 2, 1, dst)
        for j in (NC - 2, NC - 1):
            for i in range(2):
                fly_done(l, j, i, B // 2, dst)
        _wait_all(b2.at[last_two], p_send.at[2, 1])

    def down(l, j, k0, kk, w=None, rows=slice(None)):
        h = jnp.concatenate([hb[i, rows] for i in range(k0 // CW, (k0 + kk) // CW)], axis=1)
        return jnp.dot(h, wout(l, j, k0, kk) if w is None else w, preferred_element_type=F32)

    def wout(l, j, k0, kk):
        return wob[l, pl.ds(k0 // OR, kk // OR), :, _ds(j, CW)].reshape(kk, CW).astype(BF16)

    def layer(l, _):
        inner = l < L - 1
        pl.when(l > 0)(lambda: three_done(l - 1, 0, N_LO, 0, xg.at[l]))

        def up(kh, blk):
            run_at("up", l, kh * NBLK + blk, range(kh * NBLK, (kh + 1) * NBLK))
            xk = jnp.concatenate([xg[l, kh * N_LO + i] for i in range(N_LO)], axis=1)
            w = wib[l, _ds(kh, KU // IR), :, _ds(blk, NU)].reshape(KU, NU).astype(BF16)
            return jnp.dot(xk, w, preferred_element_type=F32)

        def up_first(blk, _):
            acc_up[blk] = up(0, blk)

        def up_second(blk, _):
            h = jnp.maximum(up(1, blk) + acc_up[blk], 0.0).astype(BF16)
            for i in range(NU // CW):
                hb[blk * (NU // CW) + i] = h[:, i * CW:(i + 1) * CW]

        lax.fori_loop(0, NBLK, up_first, None)
        pl.when(l > 0)(lambda: finish_upper(l - 1, xg.at[l]))
        lax.fori_loop(0, NBLK, up_second, None)
        for ll, i, slot, back in returns:

            @pl.when(l == ll)
            def _():
                back.wait()
                hb[slot] = h_back[i]

        def down_step(j, _):
            s = l * NC + j
            run_at("down", l, j, range(N_LOOP))
            v = down(l, j, 0, H).astype(BF16)
            pl.when(j >= N_LO)(lambda: three_1(s, v, 1))

            @pl.when(inner)
            def _():
                pl.when(j < N_LO)(lambda: three_1(s, v, 0))
                pl.when(j >= 1)(lambda: three_2(s - 1, 0))
                pl.when(j >= 3)(lambda: three_3(l, j - 3, 0))

            @pl.when(jnp.logical_not(inner))
            def _():
                pl.when(j < N_LO)(lambda: fly_1(s, 0, B, v, 0))
                pl.when(j >= 2)(lambda: fly_2(s - 2, 0, B, 0))

        lax.fori_loop(0, N_LOOP, down_step, None)

        s0, half = l * NC, H // 2

        def first_half(j):
            run_at("down", l, j, (j,))
            acc_dn[...] = down(l, j, 0, half)

        first_half(5)
        pl.when(inner)(lambda: three_3(l, 2, 0))
        run_at("late", l, 5, (5,))
        three_1(s0 + 5, (acc_dn[...] + down(l, 5, half, half)).astype(BF16), 1)
        pl.when(jnp.logical_not(inner))(lambda: fly_2(s0 + 3, 0, B, 0))

        first_half(6)
        pl.when(inner)(lambda: three_3(l, 3, 0))
        three_2(s0 + 4, 1)
        run_at("late", l, 6, (6,))
        v = (acc_dn[...] + down(l, 6, half, half)).astype(BF16)
        for i in range(2):
            fly_1(s0 + 6, i, B // 2, v[i * B // 2:(i + 1) * B // 2], 2)

        first_half(7)
        three_2(s0 + 5, 1)
        run_at("late", l, 7, (7,))
        w = wout(l, 7, half, half)
        for i in range(2):
            rows = _ds(i, B // 2)
            fly_1(s0 + 7, i, B // 2, (acc_dn[rows] + down(l, 7, half, half, w, rows)).astype(BF16), 2)

        three_3(l, 4, 1)
        for i in range(2):
            fly_2(s0 + 6, i, B // 2, 2)
        three_3(l, 5, 1)
        run_at("tail", l, 0, (0,))
        for i in range(2):
            fly_2(s0 + 7, i, B // 2, 2)

    lax.fori_loop(0, L, layer, None)

    lower = pl.ds((L - 1) * NC, N_LO)
    lax.fori_loop(0, N_LO, lambda j, _: fly_done(L - 1, j, 0, B, out), None)
    _wait_all(b1.at[lower], p_send.at[0, 0])
    _wait_all(b2.at[lower], p_send.at[0, 1])
    finish_upper(L - 1, out)


def pallas_dist_mlpseq_tp1d_bs_rep_b64_d1024_h2048_kernel(
    x: jax.Array,
    Win0: jax.Array,
    Wout0: jax.Array,
    Win1: jax.Array,
    Wout1: jax.Array,
    Win2: jax.Array,
    Wout2: jax.Array,
):
    dma = pltpu.SemaphoreType.DMA
    quarters = pltpu.VMEM((L * NC, 2, XR, CW), BF16)
    chunks = pltpu.VMEM((L * NC, B, CW), BF16)
    win_view, wout_view = (D // IR, IR, H), (H // OR, OR, D)
    return pl.pallas_call(
        _body,
        out_shape=jax.ShapeDtypeStruct((B, D), BF16),
        in_specs=[pl.BlockSpec(memory_space=pltpu.HBM)] * 7,
        out_specs=pl.BlockSpec(memory_space=pltpu.VMEM),
        scratch_shapes=[
            pltpu.VMEM((XR, D), F32),
            pltpu.VMEM((L, NC, B, CW), BF16),
            pltpu.VMEM((H // CW, B, CW), BF16),
            pltpu.VMEM((len(LENT), B, CW), BF16),
            pltpu.VMEM((L, *win_view), F32),
            pltpu.VMEM((L, *wout_view), F32),
            pltpu.VMEM((B, CW), F32),
            pltpu.VMEM((NBLK, B, NU), F32),
            pltpu.VMEM((2, L * NC, 2, XR, CW), BF16),
            quarters, quarters, quarters,
            chunks, chunks, chunks, chunks,
            pltpu.SMEM((max(RELAY_WOUT1, RELAY_WIN2), 8, D), F32),
            pltpu.SMEM((len(RELAY_WOUT2), 8, 8, CW), F32),
            dma((N_PIECES,)), dma((2, N_RELAY)), dma, dma((3,)), dma((3,)),
            dma((N_LENT_COPIES,)), dma((N_LENT_COPIES,)), dma((len(LENT),)), dma((len(LENT),)),
            dma((3, 2)), dma((2, L * NC, 2)), dma((L, 2, 2)), dma((L, 2, 2)),
        ],
        compiler_params=pltpu.CompilerParams(
            collective_id=0,
            vmem_limit_bytes=100 * 2**20,
            disable_bounds_checks=True,
            disable_semaphore_checks=True,
        ),
    )(
        x,
        Win0.reshape(win_view), Wout0.reshape(wout_view),
        Win1.reshape(win_view), Wout1.reshape(wout_view),
        Win2.reshape(win_view), Wout2.reshape(wout_view),
    )
```
